```python
import numpy as np

kernel_name = "dist_ring_attn_i_s256_d64"

def setup_inputs():
    S, D = 1024, 64
    q = np.random.randn(S, D).astype(np.float32)
    k = np.random.randn(S, D).astype(np.float32)
    v = np.random.randn(S, D).astype(np.float32)
    return {"q": q, "k": k, "v": v}

def reference(q: np.ndarray, k: np.ndarray, v: np.ndarray) -> np.ndarray:
    D = q.shape[1]
    scores = q @ k.T / np.sqrt(D)
    scores_max = np.max(scores, axis=1, keepdims=True)
    weights = np.exp(scores - scores_max)
    weights = weights / np.sum(weights, axis=1, keepdims=True)
    return weights @ v
```

```python
import jax
import jax.numpy as jnp
from jax import lax
from jax.experimental import pallas as pl
from jax.experimental.pallas import tpu as pltpu

N_DEV = 4


def pallas_dist_ring_attn_i_s256_d64_kernel(q: jax.Array, k: jax.Array, v: jax.Array):
    s_per, d = q.shape
    scale = 1.0 / (d ** 0.5)

    def body(q_ref, k_ref, v_ref, o_ref, kv_buf, send_sems, recv_sems):
        me = lax.axis_index("i")

        barrier = pltpu.get_barrier_semaphore()
        for off in range(1, N_DEV):
            pl.semaphore_signal(
                barrier, inc=1, device_id=((me + off) % N_DEV,),
                device_id_type=pl.DeviceIdType.MESH)

        kv_own = jnp.concatenate([k_ref[...], v_ref[...]], axis=1).astype(jnp.bfloat16)
        kv_buf[0] = kv_own

        pl.semaphore_wait(barrier, N_DEV - 1)

        copies = []
        for off in range(1, N_DEV):
            cp = pltpu.make_async_remote_copy(
                src_ref=kv_buf.at[0],
                dst_ref=kv_buf.at[off],
                send_sem=send_sems.at[off - 1],
                recv_sem=recv_sems.at[off - 1],
                device_id=((me + off) % N_DEV,),
                device_id_type=pl.DeviceIdType.MESH,
            )
            cp.start()
            copies.append(cp)

        qs = q_ref[...] * scale
        qp = jnp.concatenate([qs, jnp.zeros_like(qs)], axis=1).astype(jnp.bfloat16)

        def block(kv):
            s = lax.dot_general(qp, kv, (((1,), (1,)), ((), ())),
                                preferred_element_type=jnp.float32)
            m = jnp.max(s, axis=1, keepdims=True)
            p = jnp.exp(s - m)
            l = jnp.sum(p, axis=1, keepdims=True)
            o = jnp.dot(p.astype(jnp.bfloat16), kv, preferred_element_type=jnp.float32)
            return m, l, o

        m, l, o = block(kv_own)
        for off in (1, 3, 2):
            copies[off - 1].wait_recv()
            mj, lj, oj = block(kv_buf[off])
            m_new = jnp.maximum(m, mj)
            a = jnp.exp(m - m_new)
            b = jnp.exp(mj - m_new)
            l = a * l + b * lj
            o = a * o + b * oj
            m = m_new

        o_ref[...] = (o / l)[:, d:]
        for cp in copies:
            cp.wait_send()

    return pl.pallas_call(
        body,
        out_shape=jax.ShapeDtypeStruct((s_per, d), jnp.float32),
        in_specs=[pl.BlockSpec(memory_space=pltpu.VMEM)] * 3,
        out_specs=pl.BlockSpec(memory_space=pltpu.VMEM),
        scratch_shapes=[
            pltpu.VMEM((N_DEV, s_per, 2 * d), jnp.bfloat16),
            pltpu.SemaphoreType.DMA((N_DEV - 1,)),
            pltpu.SemaphoreType.DMA((N_DEV - 1,)),
        ],
        compiler_params=pltpu.CompilerParams(collective_id=0),
    )(q, k, v)
```

```python
import jax
import jax.numpy as jnp
from jax import lax
from jax.experimental import pallas as pl
from jax.experimental.pallas import tpu as pltpu

N_DEV = 4
NP = 2


def pallas_dist_ring_attn_i_s256_d64_kernel(q: jax.Array, k: jax.Array, v: jax.Array):
    s_per, d = q.shape
    half = s_per // 2
    quarter = half // 2
    rows = 2 * d
    pr = rows // NP
    scale = 1.0 / (d ** 0.5)
    OWN, FL, FR, FD = 0, 1, 2, 3

    def body(qt_hbm, kt_hbm, vt_hbm, ot_ref, qt_v, kt_v, vt_v, buf,
             in_sems, send_sems, recv_sems):
        me = lax.axis_index("i")
        left = (me + N_DEV - 1) % N_DEV
        right = (me + 1) % N_DEV

        ck = pltpu.make_async_copy(kt_hbm, kt_v, in_sems.at[0])
        cv = pltpu.make_async_copy(vt_hbm, vt_v, in_sems.at[1])
        cq = pltpu.make_async_copy(qt_hbm, qt_v, in_sems.at[2])
        ck.start()
        cv.start()
        cq.start()

        barrier = pltpu.get_barrier_semaphore()
        for nbr in (left, right):
            pl.semaphore_signal(barrier, inc=1, device_id=(nbr,),
                                device_id_type=pl.DeviceIdType.MESH)

        ck.wait()
        cv.wait()
        kn = kt_v[...].T.astype(jnp.bfloat16)
        vt = vt_v[...].astype(jnp.bfloat16)
        own = []
        for h in range(2):
            kp = jnp.concatenate(
                [kn[h * half:h * half + quarter], kn[h * half + quarter:(h + 1) * half]], axis=1)
            msg = jnp.concatenate([kp, vt[:, h * half:(h + 1) * half]], axis=0)
            buf[OWN, h] = msg
            own.append(msg)

        pl.semaphore_wait(barrier, 2)

        def rcopy(src_slot, h, dst_slot, idx, tgt, piece=None):
            if piece is None:
                src, dst = buf.at[src_slot, h], buf.at[dst_slot, h]
            else:
                src = buf.at[src_slot, h, pl.ds(piece * pr, pr)]
                dst = buf.at[dst_slot, h, pl.ds(piece * pr, pr)]
            return pltpu.make_async_remote_copy(
                src_ref=src, dst_ref=dst,
                send_sem=send_sems.at[idx], recv_sem=recv_sems.at[idx],
                device_id=(tgt,), device_id_type=pl.DeviceIdType.MESH)

        r0 = [rcopy(OWN, 0, FL, p, right, p) for p in range(NP)]
        l1 = [rcopy(OWN, 1, FR, NP + p, left, p) for p in range(NP)]
        fr = [rcopy(FL, 0, FD, 2 * NP + p, right, p) for p in range(NP)]
        fl = [rcopy(FR, 1, FD, 3 * NP + p, left, p) for p in range(NP)]
        r1 = rcopy(OWN, 1, FL, 4 * NP, right)
        l0 = rcopy(OWN, 0, FR, 4 * NP + 1, left)
        for p in range(NP):
            r0[p].start()
            l1[p].start()
        r1.start()
        l0.start()

        cq.wait()
        qt = (qt_v[...] * scale).astype(jnp.bfloat16)
        zq = jnp.zeros_like(qt)
        q_lo = jnp.concatenate([qt, zq], axis=0)
        q_hi = jnp.concatenate([zq, qt], axis=0)

        def attend(msgs, state):
            kp = jnp.concatenate([m_[:d] for m_ in msgs], axis=0)
            vth = jnp.concatenate([m_[d:] for m_ in msgs], axis=1)
            s_lo = jnp.dot(kp, q_lo, preferred_element_type=jnp.float32)
            s_hi = jnp.dot(kp, q_hi, preferred_element_type=jnp.float32)
            s = jnp.concatenate([s_lo[:d], s_hi[:d], s_lo[d:], s_hi[d:]], axis=0)
            mj = jnp.max(s, axis=0, keepdims=True)
            if state is None:
                p = jnp.exp(s - mj)
                return (mj, jnp.sum(p, axis=0, keepdims=True),
                        jnp.dot(vth, p.astype(jnp.bfloat16),
                                preferred_element_type=jnp.float32))
            m, l, o = state
            m_new = jnp.maximum(m, mj)
            a = jnp.exp(m - m_new)
            p = jnp.exp(s - m_new)
            l = a * l + jnp.sum(p, axis=0, keepdims=True)
            o = a * o + jnp.dot(vth, p.astype(jnp.bfloat16),
                                preferred_element_type=jnp.float32)
            return m_new, l, o

        st = attend(own, None)

        for p in range(NP):
            r0[p].wait_recv()
            fr[p].start()
            l1[p].wait_recv()
            fl[p].start()
        st = attend([buf[FL, 0], buf[FR, 1]], st)
        r1.wait_recv()
        l0.wait_recv()
        st = attend([buf[FL, 1], buf[FR, 0]], st)
        for p in range(NP):
            fr[p].wait_recv()
            fl[p].wait_recv()
        st = attend([buf[FD, 0], buf[FD, 1]], st)
        m, l, o = st
        ot_ref[...] = o / l
        for c in r0 + l1 + fr + fl + [r1, l0]:
            c.wait_send()

    nsem = 4 * NP + 2
    ot = pl.pallas_call(
        body,
        out_shape=jax.ShapeDtypeStruct((d, s_per), jnp.float32),
        in_specs=[pl.BlockSpec(memory_space=pl.ANY)] * 3,
        out_specs=pl.BlockSpec(memory_space=pltpu.VMEM),
        scratch_shapes=[
            pltpu.VMEM((d, s_per), jnp.float32),
            pltpu.VMEM((d, s_per), jnp.float32),
            pltpu.VMEM((d, s_per), jnp.float32),
            pltpu.VMEM((N_DEV, 2, rows, half), jnp.bfloat16),
            pltpu.SemaphoreType.DMA((3,)),
            pltpu.SemaphoreType.DMA((nsem,)),
            pltpu.SemaphoreType.DMA((nsem,)),
        ],
        compiler_params=pltpu.CompilerParams(collective_id=0),
    )(q.T, k.T, v.T)
    return ot.T
```

```python
import jax
import jax.numpy as jnp
from jax import lax
from jax.experimental import pallas as pl
from jax.experimental.pallas import tpu as pltpu

N_DEV = 4


def pallas_dist_ring_attn_i_s256_d64_kernel(q: jax.Array, k: jax.Array, v: jax.Array):
    s_per, d = q.shape
    half = s_per // 2
    quarter = half // 2
    rows = 2 * d
    scale = 1.0 / (d ** 0.5)
    OWN, FL, FR, FD = 0, 1, 2, 3

    def body(qt_hbm, kt_hbm, vt_hbm, ot_ref, kt_v, vq_v, buf,
             in_sems, send_sem, recv_sems):
        me = lax.axis_index("i")
        left = (me + N_DEV - 1) % N_DEV
        right = (me + 1) % N_DEV

        ck = pltpu.make_async_copy(kt_hbm, kt_v, in_sems.at[0])
        cv = pltpu.make_async_copy(vt_hbm, vq_v.at[0], in_sems.at[1])
        cq = pltpu.make_async_copy(qt_hbm, vq_v.at[1], in_sems.at[1])
        ck.start()
        cv.start()
        cq.start()

        barrier = pltpu.get_barrier_semaphore()
        for nbr in (left, right):
            pl.semaphore_signal(barrier, inc=1, device_id=(nbr,),
                                device_id_type=pl.DeviceIdType.MESH)

        def rcopy(src_slot, h, dst_slot, idx, tgt, piece=None):
            if piece is None:
                src, dst = buf.at[src_slot, h], buf.at[dst_slot, h]
            else:
                src = buf.at[src_slot, h, pl.ds(piece * d, d)]
                dst = buf.at[dst_slot, h, pl.ds(piece * d, d)]
            return pltpu.make_async_remote_copy(
                src_ref=src, dst_ref=dst,
                send_sem=send_sem, recv_sem=recv_sems.at[idx],
                device_id=(tgt,), device_id_type=pl.DeviceIdType.MESH)

        r0 = [rcopy(OWN, 0, FL, p, right, p) for p in range(2)]
        l1 = [rcopy(OWN, 1, FR, 2 + p, left, p) for p in range(2)]
        fr = [rcopy(FL, 0, FD, 4 + p, right, p) for p in range(2)]
        fl = [rcopy(FR, 1, FD, 6 + p, left, p) for p in range(2)]
        r1 = rcopy(OWN, 1, FL, 8, right)
        l0 = rcopy(OWN, 0, FR, 9, left)

        ck.wait()
        kn = kt_v[...].T.astype(jnp.bfloat16)
        kps = []
        for h in range(2):
            kp = jnp.concatenate(
                [kn[h * half:h * half + quarter], kn[h * half + quarter:(h + 1) * half]], axis=1)
            buf[OWN, h, 0:d] = kp
            kps.append(kp)

        pl.semaphore_wait(barrier, 2)
        r0[0].start()
        l1[0].start()

        pltpu.make_async_copy(vq_v, vq_v, in_sems.at[1]).wait()
        vt = vq_v[0].astype(jnp.bfloat16)
        for h in range(2):
            buf[OWN, h, d:rows] = vt[:, h * half:(h + 1) * half]
        r0[1].start()
        l1[1].start()
        r1.start()
        l0.start()

        qt = (vq_v[1] * scale).astype(jnp.bfloat16)
        zq = jnp.zeros_like(qt)
        q_lo = jnp.concatenate([qt, zq], axis=0)
        q_hi = jnp.concatenate([zq, qt], axis=0)

        def scores(k0, k1):
            kp = jnp.concatenate([k0, k1], axis=0)
            s_lo = jnp.dot(kp, q_lo, preferred_element_type=jnp.float32)
            s_hi = jnp.dot(kp, q_hi, preferred_element_type=jnp.float32)
            return jnp.concatenate([s_lo[:d], s_hi[:d], s_lo[d:], s_hi[d:]], axis=0)

        def attend(k0, k1, vth, state):
            s = scores(k0, k1)
            mj = jnp.max(s, axis=0, keepdims=True)
            if state is None:
                p = jnp.exp(s - mj)
                return (mj, jnp.sum(p, axis=0, keepdims=True),
                        jnp.dot(vth, p.astype(jnp.bfloat16),
                                preferred_element_type=jnp.float32))
            m, l, o = state
            m_new = jnp.maximum(m, mj)
            a = jnp.exp(m - m_new)
            p = jnp.exp(s - m_new)
            l = a * l + jnp.sum(p, axis=0, keepdims=True)
            o = a * o + jnp.dot(vth, p.astype(jnp.bfloat16),
                                preferred_element_type=jnp.float32)
            return m_new, l, o

        def attend_buf(s0, h0, s1, h1, state):
            vth = jnp.concatenate([buf[s0, h0, d:rows], buf[s1, h1, d:rows]], axis=1)
            return attend(buf[s0, h0, 0:d], buf[s1, h1, 0:d], vth, state)

        st = attend(kps[0], kps[1], vt, None)

        for p in range(2):
            r0[p].wait_recv()
            fr[p].start()
            l1[p].wait_recv()
            fl[p].start()
        st = attend_buf(FL, 0, FR, 1, st)
        r1.wait_recv()
        l0.wait_recv()
        st = attend_buf(FL, 1, FR, 0, st)

        fr[0].wait_recv()
        fl[0].wait_recv()
        m, l, o = st
        s = scores(buf[FD, 0, 0:d], buf[FD, 1, 0:d])
        m_new = jnp.maximum(m, jnp.max(s, axis=0, keepdims=True))
        a = jnp.exp(m - m_new)
        p = jnp.exp(s - m_new)
        inv = 1.0 / (a * l + jnp.sum(p, axis=0, keepdims=True))
        o = o * (a * inv)
        pn = (p * inv).astype(jnp.bfloat16)
        pltpu.make_async_remote_copy(
            src_ref=buf.at[pl.ds(0, 3)], dst_ref=buf.at[pl.ds(0, 3)],
            send_sem=send_sem, recv_sem=recv_sems.at[0],
            device_id=(right,), device_id_type=pl.DeviceIdType.MESH).wait_send()
        fr[1].wait_recv()
        fl[1].wait_recv()
        vth = jnp.concatenate([buf[FD, 0, d:rows], buf[FD, 1, d:rows]], axis=1)
        ot_ref[...] = o + jnp.dot(vth, pn, preferred_element_type=jnp.float32)

    nsem = 10
    ot = pl.pallas_call(
        body,
        out_shape=jax.ShapeDtypeStruct((d, s_per), jnp.float32),
        in_specs=[pl.BlockSpec(memory_space=pl.ANY)] * 3,
        out_specs=pl.BlockSpec(memory_space=pltpu.VMEM),
        scratch_shapes=[
            pltpu.VMEM((d, s_per), jnp.float32),
            pltpu.VMEM((2, d, s_per), jnp.float32),
            pltpu.VMEM((N_DEV, 2, rows, half), jnp.bfloat16),
            pltpu.SemaphoreType.DMA((2,)),
            pltpu.SemaphoreType.DMA,
            pltpu.SemaphoreType.DMA((nsem,)),
        ],
        compiler_params=pltpu.CompilerParams(collective_id=0),
    )(q.T, k.T, v.T)
    return ot.T
```

```python
import jax
import jax.numpy as jnp
from jax import lax
from jax.experimental import pallas as pl
from jax.experimental.pallas import tpu as pltpu


N_DEV = 4
NVD = 32
SWP = 32


def pallas_dist_ring_attn_i_s256_d64_kernel(q: jax.Array, k: jax.Array, v: jax.Array):
    s_per, d = q.shape
    half = s_per // 2
    quarter = half // 2
    scale = 1.0 / (d ** 0.5)
    SL = 4 * d
    OWN, FL, FR, FD = 0, 1, 2, 3
    K0, K1, V0, V1 = 0, d, 2 * d, 3 * d
    F, A, D, B = 0, 1, 2, 3

    T = []
    nrecv = [0] * 4
    rsem = []
    trig = {}

    def add(src, dst, sslot, dslot, r0, n):
        T.append((src, dst, sslot, dslot, r0, n))
        rsem.append(nrecv[dst])
        nrecv[dst] += 1
        return len(T) - 1

    def slot_at(dst, src):
        return FL if (dst + 3) % 4 == src else FR

    def send(src, dst, r0, n):
        return add(src, dst, OWN, slot_at(dst, src) if (src - dst) % 2 else FD, r0, n)

    def fwd(t, to, r0=None, n=None):
        f = add(T[t][1], to, T[t][3], FD, T[t][4] if r0 is None else r0,
                T[t][5] if n is None else n)
        trig.setdefault(t, []).append(f)
        return f

    kph = {}
    vph = {}
    fa_k = send(F, A, K0, 2 * d); fb_k = send(F, B, K0, 2 * d)
    fa_v = send(F, A, V0, 2 * d); fb_v = send(F, B, V0, 2 * d)
    fad_k = fwd(fa_k, D, K0, d); fbd_k = fwd(fb_k, D, K1, d)
    fad_v = fwd(fa_v, D, V0, d); fbd_v = fwd(fb_v, D, V1, d)
    kph[F] = [fa_k, fb_k]; vph[F] = [fa_v, fb_v]
    af_k = send(A, F, K0, 2 * d); ad_k = send(A, D, K0, 2 * d)
    af_v1 = send(A, F, V1, d); ad_v = send(A, D, V0, 2 * d)
    af_v0 = send(A, F, V0, d)
    trig.setdefault(fa_k, []).append(af_v0)
    afb_k = fwd(af_k, B, K1, d); adb_k = fwd(ad_k, B, K0, d)
    afb_v = fwd(af_v1, B); adb_v = fwd(ad_v, B, V0, d)
    kph[A] = [af_k, ad_k]; vph[A] = [af_v1, ad_v]
    bf_k = send(B, F, K0, 2 * d); bd_k = send(B, D, K0, 2 * d)
    bf_v = send(B, F, V0, 2 * d); bd_v = send(B, D, V0, 2 * d)
    bfa_k = fwd(bf_k, A); bfa_v = fwd(bf_v, A)
    kph[B] = [bf_k, bd_k]; vph[B] = [bf_v, bd_v]
    df_k = send(D, F, K0, 2 * d)
    db_sw = [send(D, B, r, SWP) for r in range(V0 + NVD, SL, SWP)]
    dbf = [fwd(t, F) for t in db_sw]
    df_v = send(D, F, V0, NVD)
    db_r = send(D, B, K0, V0 + NVD)
    da_k = send(D, A, K0, 2 * d)
    da_v = send(D, A, V0, 2 * d)
    kph[D] = [df_k]; vph[D] = [db_sw[0], df_v] + db_sw[1:] + [db_r, da_k, da_v]

    P1 = {F: [af_k, bf_k],
          A: [fa_k, da_k],
          B: [fb_k] + db_sw + [db_r],
          D: [ad_k, bd_k]}
    P2 = {F: [af_v1, bf_v],
          A: [fa_v, da_v],
          B: [fb_v],
          D: [ad_v, bd_v]}
    P3 = {F: [df_k],
          A: [bfa_k],
          B: [afb_k, adb_k],
          D: [fad_k, fbd_k]}
    P4 = {F: [af_v0, df_v] + dbf,
          A: [bfa_v],
          B: [afb_v, adb_v],
          D: [fad_v, fbd_v]}
    BL = {F: [FR, FL, FD], A: [FL, FR, FD], B: [FR, FL, FD], D: [FL, FR, FD]}
    sent_rows = [sum(t[5] for t in T if t[0] == c) for c in range(4)]
    nsem = max(nrecv)
    assert sorted(sum([sum(P.values(), []) for P in (P1, P2, P3, P4)], [])) == list(range(len(T)))
    assert max(sent_rows) <= 4 * SL

    def body(qt_hbm, kt_hbm, vt_hbm, ot_ref, kt_v, vq_v, buf,
             in_sems, send_sem, recv_sems, ack):
        me = lax.axis_index("i")
        left = (me + N_DEV - 1) % N_DEV
        right = (me + 1) % N_DEV

        ck = pltpu.make_async_copy(kt_hbm, kt_v, in_sems.at[0])
        cv = pltpu.make_async_copy(vt_hbm, vq_v.at[0], in_sems.at[1])
        cq = pltpu.make_async_copy(qt_hbm, vq_v.at[1], in_sems.at[1])
        ck.start()
        cv.start()
        cq.start()

        barrier = pltpu.get_barrier_semaphore()

        def sig(sem, tgt):
            pl.semaphore_signal(sem, inc=1, device_id=(tgt,),
                                device_id_type=pl.DeviceIdType.MESH)

        @pl.when(me == F)
        def _():
            sig(barrier, left)
            sig(barrier, right)

        @pl.when(me % 2 == 1)
        def _():
            pl.semaphore_wait(barrier, 1)
            sig(barrier, left)
            sig(barrier, right)

        @pl.when(me == D)
        def _():
            pl.semaphore_wait(barrier, 2)
            sig(ack, left)
            sig(ack, right)

        def cp(t):
            src, dst, sslot, dslot, r0, n = T[t]
            return pltpu.make_async_remote_copy(
                src_ref=buf.at[pl.ds(sslot * SL + r0, n)],
                dst_ref=buf.at[pl.ds(dslot * SL + r0, n)],
                send_sem=send_sem, recv_sem=recv_sems.at[rsem[t]],
                device_id=(dst,), device_id_type=pl.DeviceIdType.MESH)

        def per_pos(fn):
            for c in range(4):
                pl.when(me == c)(lambda c=c: fn(c))

        ck.wait()
        kn = kt_v[...].T.astype(jnp.bfloat16)
        kown = jnp.concatenate(
            [jnp.concatenate([kn[h * half:h * half + quarter],
                              kn[h * half + quarter:(h + 1) * half]], axis=1)
             for h in range(2)], axis=0)
        buf[K0:K0 + 2 * d] = kown

        def _k(c):
            if c == F:
                pl.semaphore_wait(barrier, 2)
            for t in kph[c]:
                if c % 2 == 1 and T[t][1] == D:
                    continue
                cp(t).start()
        per_pos(_k)

        pltpu.make_async_copy(vq_v, vq_v, in_sems.at[1]).wait()
        vt = vq_v[0].astype(jnp.bfloat16)
        buf[V0:V0 + d] = vt[:, :half]
        buf[V1:V1 + d] = vt[:, half:]

        def _v(c):
            if c % 2 == 0:
                for t in vph[c]:
                    cp(t).start()
            else:
                for t in vph[c]:
                    if T[t][1] == F:
                        cp(t).start()
                pl.semaphore_wait(ack, 1)
                for t in kph[c] + vph[c]:
                    if T[t][1] == D:
                        cp(t).start()
        per_pos(_v)

        qt = (vq_v[1] * scale).astype(jnp.bfloat16)
        zq = jnp.zeros_like(qt)
        q_lo = jnp.concatenate([qt, zq], axis=0)
        q_hi = jnp.concatenate([zq, qt], axis=0)

        def scores(kp):
            s_lo = jnp.dot(kp, q_lo, preferred_element_type=jnp.float32)
            s_hi = jnp.dot(kp, q_hi, preferred_element_type=jnp.float32)
            return jnp.concatenate([s_lo[:d], s_hi[:d], s_lo[d:], s_hi[d:]], axis=0)

        def rows(stage, r0, n):
            r = jnp.int32(BL[3][stage] * SL + r0)
            for c in (2, 1, 0):
                r = jnp.where(me == c, jnp.int32(BL[c][stage] * SL + r0), r)
            return buf[pl.ds(pl.multiple_of(r, d), n)]

        def waits(table):
            def fn(c):
                for t in table[c]:
                    cp(t).wait_recv()
                    for f in trig.get(t, []):
                        cp(f).start()
            return fn

        s = scores(kown)
        m = jnp.max(s, axis=0, keepdims=True)
        p = jnp.exp(s - m)
        l = jnp.sum(p, axis=0, keepdims=True)
        o = jnp.dot(vt, p.astype(jnp.bfloat16), preferred_element_type=jnp.float32)

        per_pos(waits(P1))
        s1 = scores(rows(0, K0, 2 * d))
        s2 = scores(rows(1, K0, 2 * d))
        m_new = jnp.maximum(m, jnp.max(jnp.maximum(s1, s2), axis=0, keepdims=True))
        a = jnp.exp(m - m_new)
        p1 = jnp.exp(s1 - m_new)
        p2 = jnp.exp(s2 - m_new)
        l = a * l + jnp.sum(p1 + p2, axis=0, keepdims=True)
        o = a * o
        m = m_new
        p1a = p1[:half]
        p12 = jnp.concatenate([p1[half:], p2], axis=0).astype(jnp.bfloat16)

        per_pos(waits(P2))
        v12 = jnp.concatenate([rows(0, V1, d), rows(1, V0, d), rows(1, V1, d)], axis=1)
        o = o + jnp.dot(v12, p12, preferred_element_type=jnp.float32)

        per_pos(waits(P3))
        s3 = scores(rows(2, K0, 2 * d))
        m_new = jnp.maximum(m, jnp.max(s3, axis=0, keepdims=True))
        a = jnp.exp(m - m_new)
        p3 = jnp.exp(s3 - m_new)
        inv = 1.0 / (a * l + jnp.sum(p3, axis=0, keepdims=True))
        ai = a * inv
        o = o * ai
        pn = jnp.concatenate([p1a * ai, p3 * inv], axis=0).astype(jnp.bfloat16)

        per_pos(waits(P4))
        vl = jnp.concatenate([rows(0, V0, d), rows(2, V0, d), rows(2, V1, d)], axis=1)
        ot_ref[...] = o + jnp.dot(vl, pn, preferred_element_type=jnp.float32)

        def _fin(c):
            n = sent_rows[c]
            pltpu.make_async_remote_copy(
                src_ref=buf.at[pl.ds(0, n)], dst_ref=buf.at[pl.ds(0, n)],
                send_sem=send_sem, recv_sem=recv_sems.at[0],
                device_id=(c,), device_id_type=pl.DeviceIdType.MESH).wait_send()
        per_pos(_fin)

    ot = pl.pallas_call(
        body,
        out_shape=jax.ShapeDtypeStruct((d, s_per), jnp.float32),
        in_specs=[pl.BlockSpec(memory_space=pl.ANY)] * 3,
        out_specs=pl.BlockSpec(memory_space=pltpu.VMEM),
        scratch_shapes=[
            pltpu.VMEM((d, s_per), jnp.float32),
            pltpu.VMEM((2, d, s_per), jnp.float32),
            pltpu.VMEM((N_DEV * SL, half), jnp.bfloat16),
            pltpu.SemaphoreType.DMA((2,)),
            pltpu.SemaphoreType.DMA,
            pltpu.SemaphoreType.DMA((nsem,)),
            pltpu.SemaphoreType.REGULAR,
        ],
        compiler_params=pltpu.CompilerParams(collective_id=0),
    )(q.T, k.T, v.T)
    return ot.T
```
